```python
import numpy as np

kernel_name = "dist_rope_attn_htp_bs_b2_sq512_d1024_hq8_dh128"

def setup_inputs():
    x = np.random.randn(8, 512, 1024).astype(np.float32)
    Wq = np.random.randn(1024, 4096).astype(np.float32) * 0.02
    Wk = np.random.randn(1024, 4096).astype(np.float32) * 0.02
    Wv = np.random.randn(1024, 4096).astype(np.float32) * 0.02
    Wo = np.random.randn(4096, 1024).astype(np.float32) * 0.02
    return {"x": x, "Wq": Wq, "Wk": Wk, "Wv": Wv, "Wo": Wo}

def reference(x, Wq, Wk, Wv, Wo):
    B, Sq, Hq, Dh = 8, 512, 32, 128
    inv = 1.0 / (10000.0 ** (np.arange(0, Dh, 2) / Dh))
    pos = np.arange(Sq)[:, None] * inv[None, :]
    cos = np.repeat(np.cos(pos), 2, axis=-1).astype(np.float32)
    sin = np.repeat(np.sin(pos), 2, axis=-1).astype(np.float32)
    def rot(t):
        t2 = t.reshape(B, Sq, Hq, Dh // 2, 2)
        t_r = np.stack([-t2[..., 1], t2[..., 0]], axis=-1).reshape(B, Sq, Hq, Dh)
        return t * cos[None, :, None, :] + t_r * sin[None, :, None, :]
    Q = rot((x @ Wq).reshape(B, Sq, Hq, Dh))
    K = rot((x @ Wk).reshape(B, Sq, Hq, Dh))
    V = (x @ Wv).reshape(B, Sq, Hq, Dh)
    s = np.einsum('bihd,bjhd->bhij', Q, K).astype(np.float32) * 0.08838834764831843
    s_max = s.max(axis=-1, keepdims=True)
    w = np.exp(s - s_max)
    w = w / w.sum(axis=-1, keepdims=True)
    ctx = np.einsum('bhij,bjhd->bihd', w, V).reshape(B, Sq, Hq * Dh)
    return ctx @ Wo
```

```python
import jax
import jax.numpy as jnp
from jax import lax
from jax.experimental import pallas as pl
from jax.experimental.pallas import tpu as pltpu

N_DEV = 4
BL = 2
SQ = 512
D = 1024
NH = 8
DH = 128
SCALE = 0.08838834764831843
SCHED = ((0, 0), (1, 0), (3, 0), (1, 1), (3, 1), (2, 0), (2, 1), (0, 1))


def pallas_dist_rope_attn_htp_bs_b2_sq512_d1024_hq8_dh128_kernel(x, Wq, Wk, Wv, Wo):
    def body(x_hbm, wq_hbm, wk_hbm, wv_hbm, wo_hbm, out_ref,
             stage, x_all, wqkv, wo, ctx, cos_s, sin_s, p_send, p_recv,
             ld_sem, xs_sem, xr_sem, ps_sem, pr_sem):
        me = lax.axis_index("i")

        def x_copy(d, b):
            return pltpu.make_async_remote_copy(
                src_ref=x_all.at[0, b], dst_ref=x_all.at[d, b],
                send_sem=xs_sem.at[d - 1, b], recv_sem=xr_sem.at[d - 1, b],
                device_id=((me + d) % N_DEV,), device_id_type=pl.DeviceIdType.MESH)

        def p_copy(d, b):
            return pltpu.make_async_remote_copy(
                src_ref=p_send.at[d - 1, b], dst_ref=p_recv.at[d - 1, b],
                send_sem=ps_sem.at[d - 1, b], recv_sem=pr_sem.at[d - 1, b],
                device_id=((me - d) % N_DEV,), device_id_type=pl.DeviceIdType.MESH)

        srcs = [x_hbm.at[0], x_hbm.at[1]]
        for w in (wq_hbm, wk_hbm, wv_hbm, wo_hbm):
            srcs += [w.at[pl.ds(0, SQ)], w.at[pl.ds(SQ, SQ)]]
        loads = [pltpu.make_async_copy(s, stage.at[i % 3], ld_sem.at[i % 3])
                 for i, s in enumerate(srcs)]
        for i in range(3):
            loads[i].start()
        for i in range(len(srcs)):
            loads[i].wait()
            v = stage[i % 3].astype(jnp.bfloat16)
            if i < 2:
                x_all[0, i] = v
                for d in (1, 3, 2):
                    x_copy(d, i).start()
            elif i < 8:
                j = i - 2
                wqkv[pl.ds((j % 2) * SQ, SQ), pl.ds((j // 2) * D, D)] = v
            else:
                wo[pl.ds((i - 8) * SQ, SQ), :] = v
            if i + 3 < len(srcs):
                loads[i + 3].start()

        lane = lax.broadcasted_iota(jnp.int32, (SQ, DH), 1)
        pos = lax.broadcasted_iota(jnp.int32, (SQ, DH), 0).astype(jnp.float32)
        inv = jnp.exp((lane // 2).astype(jnp.float32) * (-2.0 / DH * 9.210340371976184))
        ang = pos * inv
        even = (lane % 2) == 0
        cos_s[...] = jnp.cos(ang)
        sin_s[...] = jnp.where(even, -jnp.sin(ang), jnp.sin(ang))

        def rope(t):
            ln = lax.broadcasted_iota(jnp.int32, (SQ, DH), 1)
            sw = jnp.where((ln % 2) == 0,
                           pltpu.roll(t, DH - 1, 1), pltpu.roll(t, 1, 1))
            return t * cos_s[...] + sw * sin_s[...]

        def process(xb):
            def head(h, c):
                off = pl.multiple_of(h * DH, DH)
                q = jnp.dot(xb, wqkv[:, pl.ds(off, DH)], preferred_element_type=jnp.float32)
                k = jnp.dot(xb, wqkv[:, pl.ds(D + off, DH)], preferred_element_type=jnp.float32)
                v = jnp.dot(xb, wqkv[:, pl.ds(2 * D + off, DH)], preferred_element_type=jnp.float32)
                q = (rope(q) * SCALE).astype(jnp.bfloat16)
                k = rope(k).astype(jnp.bfloat16)
                s = lax.dot_general(q, k, (((1,), (1,)), ((), ())),
                                    preferred_element_type=jnp.float32)
                m = jnp.max(s, axis=-1, keepdims=True)
                p = jnp.exp(s - m)
                l = jnp.sum(p, axis=-1, keepdims=True)
                o = jnp.dot(p.astype(jnp.bfloat16), v.astype(jnp.bfloat16),
                            preferred_element_type=jnp.float32)
                ctx[:, pl.ds(off, DH)] = (o / l).astype(jnp.bfloat16)
                return c
            lax.fori_loop(0, NH, head, 0)
            return jnp.dot(ctx[...], wo[...], preferred_element_type=jnp.float32)

        for d, b in SCHED:
            if d > 0:
                x_copy(d, b).wait_recv()
            part = process(x_all[d, b])
            if d == 0:
                out_ref[b] = part
            else:
                p_send[d - 1, b] = part.astype(jnp.bfloat16)
                p_copy(d, b).start()

        for b in range(BL):
            acc = out_ref[b]
            for d in (1, 3, 2):
                p_copy(d, b).wait_recv()
                acc = acc + p_recv[d - 1, b].astype(jnp.float32)
            out_ref[b] = acc
        for b in range(BL):
            for d in (1, 2, 3):
                x_copy(d, b).wait_send()
                p_copy(d, b).wait_send()

    bf = jnp.bfloat16
    return pl.pallas_call(
        body,
        out_shape=jax.ShapeDtypeStruct((BL, SQ, D), jnp.float32),
        in_specs=[pl.BlockSpec(memory_space=pl.ANY)] * 5,
        out_specs=pl.BlockSpec(memory_space=pltpu.VMEM),
        scratch_shapes=[
            pltpu.VMEM((3, SQ, D), jnp.float32),
            pltpu.VMEM((N_DEV, BL, SQ, D), bf),
            pltpu.VMEM((D, 3 * D), bf),
            pltpu.VMEM((D, D), bf),
            pltpu.VMEM((SQ, D), bf),
            pltpu.VMEM((SQ, DH), jnp.float32),
            pltpu.VMEM((SQ, DH), jnp.float32),
            pltpu.VMEM((3, BL, SQ, D), bf),
            pltpu.VMEM((3, BL, SQ, D), bf),
            pltpu.SemaphoreType.DMA((3,)),
            pltpu.SemaphoreType.DMA((3, BL)),
            pltpu.SemaphoreType.DMA((3, BL)),
            pltpu.SemaphoreType.DMA((3, BL)),
            pltpu.SemaphoreType.DMA((3, BL)),
        ],
        compiler_params=pltpu.CompilerParams(vmem_limit_bytes=100 * 1024 * 1024),
    )(x, Wq, Wk, Wv, Wo)
```

```python
import jax
import jax.numpy as jnp
from jax import lax
from jax.experimental import pallas as pl
from jax.experimental.pallas import tpu as pltpu

N_DEV = 4
BL = 2
SQ = 512
D = 1024
NH = 8
DH = 128
SCALE = 0.08838834764831843
SCHED = ((1, 0), (3, 0), (1, 1), (3, 1), (2, 0), (2, 1), (0, 0), (0, 1))


def pallas_dist_rope_attn_htp_bs_b2_sq512_d1024_hq8_dh128_kernel(x, Wq, Wk, Wv, Wo):
    def body(x_hbm, wq_hbm, wk_hbm, wv_hbm, wo_hbm, out_ref,
             stage, x_all, qkv_own, wqkv, wo, ctx, cos_s, sin_s, p_send, p_recv,
             ld_sem, xs_sem, xr_sem, ps_sem, pr_sem):
        me = lax.axis_index("i")

        def x_copy(d, b):
            return pltpu.make_async_remote_copy(
                src_ref=x_all.at[0, b], dst_ref=x_all.at[d, b],
                send_sem=xs_sem.at[d - 1, b], recv_sem=xr_sem.at[d - 1, b],
                device_id=((me + d) % N_DEV,), device_id_type=pl.DeviceIdType.MESH)

        def p_copy(d, b):
            return pltpu.make_async_remote_copy(
                src_ref=p_send.at[d - 1, b], dst_ref=p_recv.at[d - 1, b],
                send_sem=ps_sem.at[d - 1, b], recv_sem=pr_sem.at[d - 1, b],
                device_id=((me - d) % N_DEV,), device_id_type=pl.DeviceIdType.MESH)

        lane = lax.broadcasted_iota(jnp.int32, (SQ, DH), 1)
        pos = lax.broadcasted_iota(jnp.int32, (SQ, DH), 0).astype(jnp.float32)
        inv = jnp.exp((lane // 2).astype(jnp.float32) * (-2.0 / DH * 9.210340371976184))
        ang = pos * inv
        cos_s[...] = jnp.cos(ang)
        sin_s[...] = jnp.where((lane % 2) == 0, -jnp.sin(ang), jnp.sin(ang))

        def rope(t):
            ln = lax.broadcasted_iota(jnp.int32, (SQ, DH), 1)
            sw = jnp.where((ln % 2) == 0,
                           pltpu.roll(t, DH - 1, 1), pltpu.roll(t, 1, 1))
            return t * cos_s[...] + sw * sin_s[...]

        def proj(xb, which, off):
            t = jnp.dot(xb, wqkv[:, pl.ds(which * D + off, DH)],
                        preferred_element_type=jnp.float32)
            if which == 0:
                t = rope(t) * SCALE
            elif which == 1:
                t = rope(t)
            return t.astype(jnp.bfloat16)

        def own_proj(which, bs):
            def head(h, c):
                off = pl.multiple_of(h * DH, DH)
                for b in bs:
                    qkv_own[b, :, pl.ds(which * D + off, DH)] = proj(x_all[0, b], which, off)
                return c
            lax.fori_loop(0, NH, head, 0, unroll=2)

        halves = lambda w: [w.at[pl.ds(0, SQ)], w.at[pl.ds(SQ, SQ)]]
        srcs = ([x_hbm.at[0]] + halves(wq_hbm) + [x_hbm.at[1]] + halves(wk_hbm)
                + halves(wv_hbm) + halves(wo_hbm))
        kinds = [("x", 0, 0), ("w", 0, 0), ("w", 0, 1), ("x", 1, 0), ("w", 1, 0),
                 ("w", 1, 1), ("w", 2, 0), ("w", 2, 1), ("o", 0, 0), ("o", 0, 1)]
        loads = [pltpu.make_async_copy(s, stage.at[i % 3], ld_sem.at[i % 3])
                 for i, s in enumerate(srcs)]
        for i in range(3):
            loads[i].start()
        for i, (kind, idx, hf) in enumerate(kinds):
            loads[i].wait()
            v = stage[i % 3].astype(jnp.bfloat16)
            if kind == "x":
                x_all[0, idx] = v
                for d in (1, 3):
                    x_copy(d, idx).start()
            elif kind == "w":
                wqkv[pl.ds(hf * SQ, SQ), pl.ds(idx * D, D)] = v
            else:
                wo[pl.ds(hf * SQ, SQ), :] = v
            if i + 3 < len(srcs):
                loads[i + 3].start()
            if i == 2:
                own_proj(0, (0,))
            elif i == 3:
                own_proj(0, (1,))
                for b in range(BL):
                    x_copy(2, b).start()
            elif i in (5, 7):
                own_proj(idx, (0, 1))

        def process(getqkv):
            def head(h, c):
                off = pl.multiple_of(h * DH, DH)
                q, k, v = getqkv(off)
                s = lax.dot_general(q, k, (((1,), (1,)), ((), ())),
                                    preferred_element_type=jnp.float32)
                m = jnp.max(s, axis=-1, keepdims=True)
                p = jnp.exp(s - m)
                l = jnp.sum(p, axis=-1, keepdims=True)
                o = jnp.dot(p.astype(jnp.bfloat16), v,
                            preferred_element_type=jnp.float32)
                ctx[:, pl.ds(off, DH)] = (o / l).astype(jnp.bfloat16)
                return c
            lax.fori_loop(0, NH, head, 0, unroll=2)
            return jnp.dot(ctx[...], wo[...], preferred_element_type=jnp.float32)

        for d, b in SCHED:
            if d > 0:
                x_copy(d, b).wait_recv()
                xb = x_all[d, b]
                part = process(lambda off: [proj(xb, w, off) for w in range(3)])
                p_send[d - 1, b] = part.astype(jnp.bfloat16)
                p_copy(d, b).start()
            else:
                acc = process(lambda off: [qkv_own[b, :, pl.ds(w * D + off, DH)]
                                           for w in range(3)])
                for dd in (1, 3, 2):
                    p_copy(dd, b).wait_recv()
                    acc = acc + p_recv[dd - 1, b].astype(jnp.float32)
                out_ref[b] = acc
        for b in range(BL):
            for d in (1, 2, 3):
                x_copy(d, b).wait_send()
                p_copy(d, b).wait_send()

    bf = jnp.bfloat16
    return pl.pallas_call(
        body,
        out_shape=jax.ShapeDtypeStruct((BL, SQ, D), jnp.float32),
        in_specs=[pl.BlockSpec(memory_space=pl.ANY)] * 5,
        out_specs=pl.BlockSpec(memory_space=pltpu.VMEM),
        scratch_shapes=[
            pltpu.VMEM((3, SQ, D), jnp.float32),
            pltpu.VMEM((N_DEV, BL, SQ, D), bf),
            pltpu.VMEM((BL, SQ, 3 * D), bf),
            pltpu.VMEM((D, 3 * D), bf),
            pltpu.VMEM((D, D), bf),
            pltpu.VMEM((SQ, D), bf),
            pltpu.VMEM((SQ, DH), jnp.float32),
            pltpu.VMEM((SQ, DH), jnp.float32),
            pltpu.VMEM((3, BL, SQ, D), bf),
            pltpu.VMEM((3, BL, SQ, D), bf),
            pltpu.SemaphoreType.DMA((3,)),
            pltpu.SemaphoreType.DMA((3, BL)),
            pltpu.SemaphoreType.DMA((3, BL)),
            pltpu.SemaphoreType.DMA((3, BL)),
            pltpu.SemaphoreType.DMA((3, BL)),
        ],
        compiler_params=pltpu.CompilerParams(vmem_limit_bytes=100 * 1024 * 1024),
    )(x, Wq, Wk, Wv, Wo)
```
